```python
import numpy as np

kernel_name = "dist_sparse_attn_strided_qseq_b1_sq1024_skv1024_hq8_dh128"

def setup_inputs():
    x = np.random.randn(1, 4096, 1024).astype(np.float32)
    Wq = np.random.randn(1024, 4096).astype(np.float32) * 0.02
    K_ext = np.random.randn(1, 1024, 32, 128).astype(np.float32)
    V_ext = np.random.randn(1, 1024, 32, 128).astype(np.float32)
    Wo = np.random.randn(4096, 1024).astype(np.float32) * 0.02
    return {"x": x, "Wq": Wq, "K_ext": K_ext, "V_ext": V_ext, "Wo": Wo}

def reference(x, Wq, K_ext, V_ext, Wo):
    B, Sq, Skv, Hq, Dh = 1, 4096, 1024, 32, 128
    Q = (x @ Wq).reshape(B, Sq, Hq, Dh)
    qb = (np.arange(Sq) // 64)[:, None]
    kb = (np.arange(Skv) // 64)[None, :]
    mask = (qb == kb) | ((kb % 4) == (qb % 4))
    scores = np.einsum('bihd,bjhd->bhij', Q, K_ext).astype(np.float32) * 0.08838834764831843
    scores = np.where(mask[None, None, :, :], scores, -1e9)
    scores_max = scores.max(axis=-1, keepdims=True)
    w = np.exp(scores - scores_max)
    row_keep = mask.any(axis=1)
    w_sum = np.where(row_keep[None, None, :, None], w.sum(axis=-1, keepdims=True), 1.0)
    w = w / w_sum
    w = np.where(row_keep[None, None, :, None], w, 0.0)
    ctx = np.einsum('bhij,bjhd->bihd', w, V_ext).reshape(B, Sq, Hq * Dh)
    return ctx @ Wo
```

```python
import jax
import jax.numpy as jnp
from jax import lax
from jax.experimental import pallas as pl
from jax.experimental.pallas import tpu as pltpu

F32 = jnp.float32
BF16 = jnp.bfloat16
QK_SCALE = 0.08838834764831843 * 1.4426950408889634

OWN, OTHER = 0, 1


T_Q, T_ATT, T_DOT = 0.62, 0.18, 0.352
T_WAIT = 0.15
T_START = 15.1
T_KV = 21.8
T_CHUNK = (15.4, 26.4, 37.9, 48.5)
T_LAST = (98.5, 110.0)
T_WO, T_BLOCK = 55.3, 5.45
CREDIT = 0.65
RUSH = (("o_a", 0), ("o_b", 0), ("o_c", 0), ("o_a", 1))
QUIET = 0.35
ATT_EVERY = (0.25, 0.15, 0.21, 0.16, 0.14)


FEEDS = ({0: 1, 3: 1}, {2: 1, 3: -1}, {1: 1, 3: 1}, {0: 1, 2: 1}, {0: -1, 1: 1}, {3: 1}, {0: 1})
OWN_ORDER = (1, 3, 2, 4, 5, 0, 6)


def _feeders(k):
    return [i for i in OWN_ORDER if k in FEEDS[i]]


def _completed(i):
    return [k for k in FEEDS[i] if _feeders(k)[-1] == i]


def _start_up():
    q = lambda rs, ps: [("q", OWN, OWN, r, p) for r in rs for p in ps]
    prep = lambda what, i: [(f"prep_{what}", OWN, i, c) for c in range(4)]
    ops = [(f"load_{what}", i) for i in range(4) for what in ("x0", "wq0")]
    ops.insert(2, ("barrier_signal",))
    ops += [("load_x", 1), ("load_wq", 1), ("load_x", 2)]
    for i in range(4):
        ops += [("wait_x0", i), ("cvt_x0", i)] + [("barrier_wait",)] * (i == 0) + [("send_x0", i)]
        ops += [("wait_wq0", i), ("cvt_wq0", i), ("send_wq0", i)]
    ops += prep("x", 0) + prep("wq", 0) + q([0], [0])
    ops += [("wait_x", 1), ("load_wq", 2)] + prep("x", 1) + q([1], [0])
    ops += [("wait_wq", 1), ("load_x", 3), ("send_x", 1)] + prep("wq", 1) + q([0, 1], [1])
    ops += [("wait_x", 2), ("load_wq", 3), ("send_wq", 1)] + prep("x", 2) + q([2], [0, 1])
    ops += [("wait_wq", 2), ("load_kv", OWN, 0), ("send_x", 2)] + prep("wq", 2) + q([0, 1], [2])
    ops += [("wait_x", 3), ("load_kv", OWN, 1), ("send_wq", 2)] + q([2], [2]) + prep("x", 3) + q([3], [0, 1])
    ops += [("wait_wq", 3), ("load_kv", OWN, 2), ("send_x", 3)] + q([3], [2]) + prep("wq", 3) + q([0], [3])
    return ops


def _schedule():
    R = range(4)
    ops = _start_up()
    kv = lambda verb, g, ps: [(f"{verb}_kv", g, p) for p in ps]
    events = [(T_CHUNK[0], kv("wait", OWN, [0]) + kv("load", OWN, [3]) + [("load_wo", 0), ("send_wq", 3)]
               + kv("load", OTHER, [0])),
              (T_KV, kv("wait", OWN, [1, 2]) + kv("load", OTHER, [1, 2]) + [("load_wo", 1)]),
              (T_CHUNK[1], kv("wait", OWN, [3]) + [("wait_wo", 0)] + kv("load", OTHER, [3]) + [("load_wo", 2), ("load_wo", 3)]),
              (T_CHUNK[2], kv("wait", OTHER, [0, 1, 2]) + [("wait_wo", 1), ("send_wo", 0), ("send_wo", 1)]),
              (T_CHUNK[3], kv("wait", OTHER, [3]) + [("wait_wo", 2), ("wait_wo", 3), ("send_wo", 2), ("send_wo", 3)]),
              (T_WO + T_BLOCK, [("send_wo", k) for k in range(4, 8)])]
    events += [(T_CHUNK[i], [("recv_x", i), ("recv_wq", i)]) for i in R]
    events += [(T_WO + T_BLOCK * k, [("recv_wo", k)]) for k in range(8)]
    events += [(T_WO + T_BLOCK * 5, [("recv_part", 0)]), (T_WO + T_BLOCK * 7, [("recv_part", 1)]),
               (T_LAST[0], [("recv_part", 2)]), (T_LAST[1], [("recv_part", 3)])]
    events.sort(key=lambda e: e[0])

    parts = lambda *op: [(*op, c) for c in R]
    urgent, ready = set(), []
    vpu, att, mm, after = {}, {}, {}, {}
    for i in R:
        for what in ("wq", "x") if i == 3 else ("x", "wq"):
            for c in R:
                vpu[f"prep_{what}", OTHER, i, c] = [(f"recv_{what}", i)]
    for j in R:
        for c in R:
            vpu["cvt_wo", j, c] = [("wait_wo", j)]

    blocks = {"o_a": [2], "o_b": [1], "o_c": [0, 3]}

    def add_q(s, g, r, p):
        mm["q", s, g, r, p] = parts("prep_x", s, r) + parts("prep_wq", g, p)
        for h in (2 * p, 2 * p + 1):
            att["att", s, g, r, h] = [("q", s, g, r, p), ("wait_kv", g, p)] + [("att", s, OWN, r, h)] * g

    def add_o(s, j):
        for c in range(2):
            rows = [("att", s, OTHER, r, h) for r in (2 * c, 2 * c + 1) for h in range(8)]
            mm["o_a", s, j, c] = rows + [("recv_wo", 2 * j)] + [("o_c", s, j - 1, c)] * (j > 0)
        for c in range(2):
            mm["o_b", s, j, c] = [("o_a", s, j, c), ("recv_wo", 2 * j + 1)]
        for c in range(2):
            mm["o_c", s, j, c] = [("o_b", s, j, c)]
            for step, ks in blocks.items():
                after[step, s, j, c] = [("send_part", j, k, c) for k in ks]
        urgent.update([("o_c", s, j, 1)] + [(step, s, 0, c) for step, c in RUSH])

    for j in R:
        add_o(OTHER, j)
    for p in R:
        for r in R:
            add_q(OWN, OWN, r, p)
    for i in R:
        for r, p in [(r, i) for r in range(i)]:
            add_q(OTHER, OTHER, r, p)
        for p in R:
            add_q(OTHER, OWN, i, p)
        for p in range(i + 1):
            add_q(OTHER, OTHER, i, p)
    att = dict(sorted(att.items(), key=lambda kv: -kv[0][1]))
    for p in R:
        for r in R:
            add_q(OWN, OTHER, r, p)
    heads = [("att", OWN, OTHER, r, h) for r in R for h in range(8)]
    for half in range(2):
        for n, i in enumerate(OWN_ORDER):
            mm["own", half, i] = (heads + [("o_c", OTHER, 2 * half + 1, 0)] + [("own", 0, i)] * half
                                  + [("own", half, OWN_ORDER[n - 1])] * (n > 0))

    cost = lambda op: {"q": T_Q, "att": T_ATT, "o_a": 3 * T_DOT, "own": 3.5 * T_DOT}.get(op[0], 2 * T_DOT)
    needs = {**mm, **att}
    settled, fresh = set(ops), set()
    mm = {op: need for op, need in mm.items() if op not in settled}
    now, credit = T_START - 3 * T_Q, 0.0

    def take(pool, known, rows=(OWN, OTHER)):
        for op, need in pool.items():
            if all(n in known for n in need) and (pool is vpu or op[0] == "own" and len(rows) == 2 or op[0] != "own" and op[1] in rows):
                del pool[op]
                return op

    def issue(op):
        fresh.add(op)
        ops.append(("complete", *[n for n in needs.get(op, ()) if not n[0] == op[0] == "own"]))
        if op[0] in ("o_a", "o_b") and ("prep_wo", op[0], op[2]) not in ops:
            ops.append(("prep_wo", op[0], op[2]))
        if op[0] == "own":
            _, half, i = op
            ops.extend([("prep_own", half, i)] + [("prep_ctx", i)] * (half == 0))
            here = tuple(("recv_part", 2 * half + e) in settled for e in range(2))
            for j, k, c in [(2 * half + e, k, c) for e in range(2) if not here[e] for k in _completed(i) for c in range(2)]:
                vpu["finish", j, k, c] = needs["finish", j, k, c] = [("recv_part", j), op]
            op += (here,)
        ops.append(op)
        if op[0] == "o_b" and ("prep_wo", "o_c", op[2]) not in ops:
            ops.append(("prep_wo", "o_c", op[2]))

    def send_ready():
        for op in [op for op in ready if op != ops[-1]]:
            ops.extend(after[op])
            ready.remove(op)

    while vpu or att or mm:
        while events and events[0][0] <= now:
            waits = events.pop(0)[1]
            assert all(("cvt_wo", w[1] // 2, c) not in vpu for w in waits if w[0] == "send_wo" for c in R)
            send_ready()
            ops.extend(waits)
            settled.update(waits)
            now += T_WAIT
        every = ATT_EVERY[sum(now >= t for t in (T_KV, *T_CHUNK[1:]))]
        quiet = events and events[0][0] - now < QUIET
        pools = (att, mm) if credit >= every and not quiet else (mm, att)
        hurry = now >= T_CHUNK[3] and any(op[1] == OTHER for op in att)
        first = take({op: mm[op] for op in mm if op in after}, settled | fresh.intersection(after))
        short = urgent.intersection(ready) or (not first and take({op: mm[op] for op in mm if op in after}, settled | fresh))
        op = (short and take(att, settled)) or first
        mm.pop(op, None)
        op = op or hurry and (take(pools[0], settled, [OTHER]) or take(pools[1], settled, [OTHER]))
        op = op or take(pools[0], settled) or take(pools[1], settled)
        if op is None:
            step = take(vpu, settled | fresh)
            if step is not None:
                issue(step)
            elif fresh:
                settled |= fresh
                fresh = set()
            else:
                now = events[0][0]
            continue
        settled |= fresh
        fresh = set()
        issue(op)
        if urgent.intersection(ready):
            send_ready()
        ready.extend([op] * (op in after))
        if op in urgent and not any(all(n in settled for n in need) for need in att.values()):
            ops.append(("complete", op))
            send_ready()
        now += cost(op)
        credit = max(credit - every, 0.0) if op[0] == "att" else min(credit + cost(op), CREDIT)
        for _ in range(0 if events and events[0][0] <= now else 3 if op[0] == "own" else round(cost(op) / T_ATT)):
            step = take(vpu, settled)
            if step is not None:
                issue(step)
    assert not events and not ready
    return ops + [("complete", *needs), ("drain",)]


def _sums_lhs(a11, a12, a21, a22):
    return (a11 + a22, a21 + a22, a11 + a12, a21 - a11, a12 - a22)


def _sums_rhs(b11, b12, b21, b22):
    return (b11 + b22, b12 - b22, b21 - b11, b11 + b12, b21 + b22)


def _dot(a, b):
    return lax.dot_general(a, b, (((1,), (0,)), ((), ())), preferred_element_type=F32)


class _Packed:
    def __init__(self, ref):
        self.ref = ref
        self.words = ref.bitcast(jnp.uint32)

    def __getitem__(self, idx):
        *lead, (start, size) = idx
        return pltpu.bitcast(self.words[(*lead, pl.ds(start // 2, size // 2), slice(None))], BF16)

    def __setitem__(self, idx, value):
        *lead, rows = idx
        self.ref[(*lead, pl.ds(*rows), slice(None))] = value.astype(BF16)

    def wide(self, *idx):
        *lead, rows = idx
        return _side_by_side(self[(*lead, slice(None), rows)])


def _side_by_side(blocks):
    n, rows, cols = blocks.shape
    flat = lax.reshape(blocks, (n * rows, cols))
    return lax.concatenate([lax.slice(flat, (c * rows, 0), ((c + 1) * rows, cols)) for c in range(n)], 1)


def _body(x_hbm, wq_hbm, k_hbm, v_hbm, wo_hbm, out_ref,
          xf, wqf, wof, kf, vf,
          x_snd, x_rcv, wq_snd, wq_rcv, wo_snd, wo_rcv, pt_snd, pt_rcv,
          xa, wqb, wob, qs, ca, cc, wc, acc, of,
          x_sem, wq_sem, wo_sem, kv_sem,
          sent_sem, xr_sem, wqr_sem, wor_sem, ptr_sem):
    me = lax.axis_index("i")
    peer_rows = me ^ 1
    peer_heads = 3 - me

    def remote(src, dst, ssem, rsem, dev):
        return pltpu.make_async_remote_copy(
            src_ref=src, dst_ref=dst, send_sem=ssem, recv_sem=rsem,
            device_id=(dev,), device_id_type=pl.DeviceIdType.MESH)

    def slab(i):
        return pl.ds(256 * i, 256)

    def x0_copy(i):
        return pltpu.make_async_copy(x_hbm.at[:, 0, :, slab(i)], xf.at[0, :, :, slab(i)], x_sem.at[4 + i])

    def wq0_copy(i):
        return pltpu.make_async_copy(wq_hbm.at[slab(i), slab(0)], wqf.at[0, slab(i)], wq_sem.at[4 + i])

    def x_copy(r):
        return pltpu.make_async_copy(x_hbm.at[:, r], xf.at[r], x_sem.at[r])

    def wq_copy(p):
        return pltpu.make_async_copy(wq_hbm.at[:, slab(p)], wqf.at[p], wq_sem.at[p])

    def wo_copy(j):
        return pltpu.make_async_copy(wo_hbm.at[:, slab(j)], wof.at[j], wo_sem.at[j])

    def kv_copies(g, p):
        head0 = 8 * (me if g == OWN else peer_heads) + 2 * p
        return [
            pltpu.make_async_copy(src.at[:, :, :, head0 + e, :], dst.at[8 * g + 2 * p + e],
                                  kv_sem.at[4 * g + p])
            for e in range(2) for src, dst in ((k_hbm, kf), (v_hbm, vf))
        ]

    def x0_send(i):
        idx = (0, i // 2, pl.ds(2 * (i % 2), 2))
        return remote(x_snd.at[idx], x_rcv.at[idx], sent_sem.at[0], xr_sem.at[0], peer_rows)

    def wq0_send(i):
        idx = (0, slice(None), slab(i))
        return remote(wq_snd.at[idx], wq_rcv.at[idx], sent_sem.at[1], wqr_sem.at[0], peer_heads)

    def x_send(r):
        return remote(x_snd.at[r], x_rcv.at[r], sent_sem.at[0], xr_sem.at[r], peer_rows)

    def wq_send(p):
        return remote(wq_snd.at[p], wq_rcv.at[p], sent_sem.at[1], wqr_sem.at[p], peer_heads)

    def wo_send(k):
        return remote(wo_snd.at[k], wo_rcv.at[k], sent_sem.at[2], wor_sem.at[k], peer_heads)

    def pt_send(j, *block):
        return remote(pt_snd.at[(j, *block)], pt_rcv.at[(j, *block)], sent_sem.at[3], ptr_sem.at[j], peer_rows)

    xs, xr, wqs, wqr, wos, wor, pts, ptr = map(
        _Packed, (x_snd, x_rcv, wq_snd, wq_rcv, wo_snd, wo_rcv, pt_snd, pt_rcv))
    xa, wqb, wob, qs, ca, cc, wc = map(_Packed, (xa, wqb, wob, qs, ca, cc, wc))
    up, down, both = (0, 128), (128, 128), (0, 256)

    latest = []

    def tie(value):
        zero = pltpu.bitcast(latest[-1], jnp.uint32) & (me // 4).astype(jnp.uint32)
        bits = pltpu.bitcast(value, jnp.uint32).reshape(-1, 8, 128) | zero
        return pltpu.bitcast(bits.reshape(value.shape), F32)

    def cvt_x0(i):
        for e in range(2):
            cols = pl.ds(256 * i + 128 * e, 128)
            xs[0, i // 2, 2 * (i % 2) + e, both] = xf[0, :, :, cols].reshape(256, 128)

    def cvt_wq0(i):
        for e in range(2):
            wqs[0, e, (256 * i, 256)] = wqf[0, slab(i), pl.ds(128 * e, 128)] * QK_SCALE

    def prep_x(s, r, c):
        if s == OWN:
            left = xf[r, :, :, pl.ds(128 * c, 128)].reshape(256, 128)
            right = xf[r, :, :, pl.ds(512 + 128 * c, 128)].reshape(256, 128)
            if r > 0:
                xs[r, 0, c, both] = left
                xs[r, 1, c, both] = right
        else:
            left, right = xr[r, 0, c, both].astype(F32), xr[r, 1, c, both].astype(F32)
        for i, v in enumerate(_sums_lhs(left[:128], right[:128], left[128:], right[128:])):
            xa[s, r, i, c, up] = v

    def prep_wq(g, p, c):
        lo, hi = (128 * c, 128), (512 + 128 * c, 128)
        if g == OWN:
            b = [wqf[p, pl.ds(*rows), pl.ds(128 * e, 128)] * QK_SCALE for rows in (lo, hi) for e in range(2)]
            if p > 0:
                for n, v in enumerate(b):
                    wqs[p, n % 2, (lo, hi)[n // 2]] = v
        else:
            b = [wqr[p, e, rows].astype(F32) for rows in (lo, hi) for e in range(2)]
        for i, v in enumerate(_sums_rhs(*b)):
            wqb[g, p, i, lo] = v

    def cvt_wo(j, c):
        rows = (256 * c, 256)
        for e in range(2):
            wos[2 * j + e, rows] = tie(wof[j, slab(c), pl.ds(128 * e, 128)])

    deep = (0, 1024)

    def prep_wo(step, j):
        b11, b12 = wof[j, :, 0:128], wof[j, :, 128:256]
        b21 = wor[2 * j, deep].astype(F32)
        if step == "o_a":
            wob[j, 2, deep] = b21 - b11
            wob[j, 3, deep] = b11 + b12
            return
        b22 = wor[2 * j + 1, deep].astype(F32)
        if step == "o_b":
            wob[j, 1, deep] = b12 - b22
        else:
            wob[j, 0, deep] = b11 + b22
            wob[j, 4, deep] = b21 + b22

    def q_proj(s, g, r, p):
        xp = xs if s == OWN else xr
        wp = wqs if g == OWN else wqr
        h = 8 * g + 2 * p
        k = (0, 512)
        products = {
            2: lambda: _dot(xa.wide(s, r, 1, up), wp[p, 0, k]),
            3: lambda: _dot(xp.wide(r, 0, up), wqb[g, p, 1, k]),
            4: lambda: _dot(xp.wide(r, 1, down), wqb[g, p, 2, k]),
            5: lambda: _dot(xa.wide(s, r, 2, up), wp[p, 1, (512, 512)]),
        }
        first, second = ((4, 3), (2, 5)) if s > g or (s == g and r > p) else ((2, 5), (4, 3))
        m = {n: products[n]() for n in first}
        latest.append(m[first[0]][:8])
        yield
        m[second[0]] = products[second[0]]()
        qs[s, r, h, down] = m[2] + m[4]
        m[second[1]] = products[second[1]]()
        qs[s, r, h + 1, up] = m[3] + m[5]
        c11, c22 = m[4] - m[5], m[3] - m[2]
        m1 = _dot(xa.wide(s, r, 0, up), wqb[g, p, 0, k])
        c22 = c22 + m1
        qs[s, r, h, up] = c11 + m1 + _dot(xa.wide(s, r, 4, up), wqb[g, p, 4, k])
        c22 = c22 + _dot(xa.wide(s, r, 3, up), wqb[g, p, 3, k])
        yield
        qs[s, r, h + 1, down] = c22

    def attention(s, g, r, h):
        k = kf[8 * g + h, :, r].reshape(256, 128).astype(BF16)
        w = []
        for part in (up, down):
            sc = lax.dot_general(qs[s, r, 8 * g + h, part], k, (((1,), (1,)), ((), ())), preferred_element_type=F32)
            latest.append(sc[:8, :128])
            w.append(jnp.exp2(sc - jnp.max(sc, axis=1, keepdims=True)).astype(BF16))
        yield
        v = vf[8 * g + h, :, r].reshape(256, 128).astype(BF16)
        ctx = []
        for part in w:
            total = jnp.sum(part.astype(F32), axis=1, keepdims=True)
            inv = pl.reciprocal(total, approx=True)
            inv = inv * (2.0 - total * inv)
            ctx.append(_dot(part, v) * inv)
        top, bot = ctx
        rows = (128 * r, 128)
        if g == OWN:
            yield
            ca[s, 5, h, rows] = top
            ca[s, 6, h, rows] = bot
            ca[s, 3, h, rows] = bot - top
        else:
            sums = _sums_lhs(ca[s, 5, h, rows].astype(F32), top, ca[s, 6, h, rows].astype(F32), bot)
            sums = {i: sums[i].astype(BF16) for i in (0, 1, 2, 4)}
            yield
            for i, v in sums.items():
                ca[s, i, h, rows] = v
            ca[s, 7, h, rows] = bot

    def o_a(s, j, c):
        rows = (256 * c, 256)
        m2 = _dot(ca.wide(s, 1, rows), wos[2 * j, deep])
        latest.append(m2[:8])
        m4 = _dot(ca.wide(s, 7, rows), wob[j, 2, deep])
        pts[j, 2, c, both] = m2 + m4
        m6 = _dot(ca.wide(s, 3, rows), wob[j, 3, deep])
        acc[c, 0] = m4
        yield
        acc[c, 1] = m6 - m2

    def o_b(s, j, c):
        rows = (256 * c, 256)
        m5 = _dot(ca.wide(s, 2, rows), wor[2 * j + 1, deep])
        latest.append(m5[:8])
        acc[c, 0] = acc[c, 0] - m5
        m3 = _dot(ca.wide(s, 5, rows), wob[j, 1, deep])
        c22 = acc[c, 1] + m3
        yield
        pts[j, 1, c, both] = m3 + m5
        acc[c, 1] = c22

    def o_c(s, j, c):
        rows = (256 * c, 256)
        m1 = _dot(ca.wide(s, 0, rows), wob[j, 0, deep])
        latest.append(m1[:8])
        pts[j, 3, c, both] = acc[c, 1] + m1
        c11 = acc[c, 0] + m1 + _dot(ca.wide(s, 4, rows), wob[j, 4, deep])
        yield
        pts[j, 0, c, both] = c11

    lhs_slot = (0, 1, 5, 7, 2, 3, 4)

    def rhs(i, j, rows):
        if i in (1, 4):
            return wos[2 * j, rows] if i == 1 else wor[2 * j + 1, rows]
        return wob[j, {0: 0, 2: 1, 3: 2, 5: 3, 6: 4}[i], rows]

    def prep_ctx(i):
        for h in range(4):
            quarters = [ca[OWN, lhs_slot[i], h + 4 * e, (256 * c, 256)].astype(F32) for c in range(2) for e in range(2)]
            for n, v in enumerate(_sums_lhs(*quarters)):
                cc[i, n, h, both] = v

    def prep_own(half, i):
        quarters = [rhs(i, 2 * half + e, (512 * c, 512)).astype(F32) for c in range(2) for e in range(2)]
        for n, v in enumerate(_sums_rhs(*quarters)):
            wc[half, i, n, (0, 512)] = v

    def own(half, i, here):
        def feed(c, e, value):
            j = 2 * half + e
            for k, sign in FEEDS[i].items():
                if _feeders(k)[0] == i:
                    total = value if sign > 0 else -value
                else:
                    total = of[j, k, c] + value if sign > 0 else of[j, k, c] - value
                if here[e] and k in _completed(i):
                    finish(j, k, c, total)
                else:
                    of[j, k, c] = total

        def plain(c):
            return _side_by_side(ca[OWN, lhs_slot[i], pl.ds(4 * c, 4), (256 * c, 256)])

        k = (0, 512)
        m4 = _dot(plain(1), wc[half, i, 2, k])
        latest.append(m4[:8])
        m3 = _dot(plain(0), wc[half, i, 1, k])
        m2 = _dot(cc.wide(i, 1, both), rhs(i, 2 * half, k))
        feed(1, 0, m2 + m4)
        c22 = m3 - m2
        m5 = _dot(cc.wide(i, 2, both), rhs(i, 2 * half + 1, (512, 512)))
        feed(0, 1, m3 + m5)
        c11 = m4 - m5
        m1 = _dot(cc.wide(i, 0, both), wc[half, i, 0, k])
        c22 = c22 + m1
        feed(0, 0, c11 + m1 + _dot(cc.wide(i, 4, both), wc[half, i, 4, k]))
        c22 = c22 + _dot(cc.wide(i, 3, both), wc[half, i, 3, k])
        yield
        feed(1, 1, c22)

    def finish(j, k, c, value=None):
        total = ((tie(of[j, k, c]) if value is None else value) + ptr[j, k, c, both].astype(F32)).astype(BF16)
        for e in range(2):
            for a in range(2):
                rows = pl.ds(512 * (k // 2) + 256 * a + 64 * (2 * c + e), 64)
                out_ref[rows, pl.ds(256 * j + 128 * (k % 2), 128)] = total[128 * e + 64 * a:128 * e + 64 * a + 64]

    def barrier_signal():
        for dev in (peer_rows, peer_heads):
            pl.semaphore_signal(pltpu.get_barrier_semaphore(), inc=1, device_id=(dev,),
                                device_id_type=pl.DeviceIdType.MESH)

    def drain():
        for n, (src, dst) in enumerate(((x_snd, x_rcv), (wq_snd, wq_rcv), (wo_snd, wo_rcv), (pt_snd, pt_rcv))):
            remote(src, dst, sent_sem.at[n], xr_sem.at[0], peer_rows).wait_send()

    compute = dict(cvt_x0=cvt_x0, cvt_wq0=cvt_wq0, prep_x=prep_x, prep_wq=prep_wq, cvt_wo=cvt_wo,
                   prep_wo=prep_wo, q=q_proj, att=attention,
                   o_a=o_a, o_b=o_b, o_c=o_c, prep_ctx=prep_ctx, prep_own=prep_own, own=own, finish=finish, drain=drain, barrier_signal=barrier_signal,
                   barrier_wait=lambda: pl.semaphore_wait(pltpu.get_barrier_semaphore(), 2))
    local = dict(x0=x0_copy, wq0=wq0_copy, x=x_copy, wq=wq_copy, wo=wo_copy, kv=kv_copies)
    sends = dict(x0=x0_send, wq0=wq0_send, x=x_send, wq=wq_send, wo=wo_send, part=pt_send)
    running = {}
    ops = _schedule()
    for n, (op, *args) in enumerate(ops):
        kind, _, what = op.partition("_")
        if op == "complete":
            for key in args:
                list(running.pop(key, ()))
        elif op in compute:
            step = compute[op](*args)
            if step is not None:
                stop_ahead = ops[n + 1][0] not in compute and ops[n + 1][0] != "complete"
                next(step)
                if op == "q" and stop_ahead:
                    next(step)
                for key in list(running):
                    if not stop_ahead:
                        list(running.pop(key))
                    elif next(running[key], "done") == "done":
                        del running[key]
                if stop_ahead or op == "att":
                    running[(op, *args[:2 if op == "own" else 4])] = step
                else:
                    list(step)
        elif kind in ("load", "wait"):
            copies = local[what](*args)
            for copy in copies if what == "kv" else [copies]:
                copy.start() if kind == "load" else copy.wait()
        elif kind == "send":
            if what == "part":
                list(running.pop((("o_c", "o_b", "o_a", "o_c")[args[1]], OTHER, args[0], args[2]), ()))
            sends[what](*args).start()
        else:
            assert kind == "recv", op
            sends[what](*args).wait_recv()


def pallas_dist_sparse_attn_strided_qseq_b1_sq1024_skv1024_hq8_dh128_kernel(
    x: jax.Array,
    Wq: jax.Array,
    K_ext: jax.Array,
    V_ext: jax.Array,
    Wo: jax.Array,
):
    vmem = pltpu.VMEM
    dma = pltpu.SemaphoreType.DMA

    def packed(*shape):
        return vmem((*shape, 128), BF16)

    hbm = pl.BlockSpec(memory_space=pltpu.HBM)
    out = pl.pallas_call(
        _body,
        out_shape=jax.ShapeDtypeStruct((1024, 1024), BF16),
        in_specs=[hbm] * 5,
        out_specs=pl.BlockSpec(memory_space=vmem),
        scratch_shapes=[
            vmem((4, 4, 64, 1024), F32),
            vmem((4, 1024, 256), F32),
            vmem((4, 1024, 256), F32),
            vmem((16, 4, 4, 64, 128), F32),
            vmem((16, 4, 4, 64, 128), F32),
            *[packed(4, 2, 4, 256)] * 2,
            *[packed(4, 2, 1024)] * 2,
            *[packed(8, 1024)] * 2,
            *[packed(4, 4, 2, 256)] * 2,
            packed(2, 4, 5, 4, 128),
            packed(2, 4, 5, 512),
            packed(4, 5, 1024),
            packed(2, 4, 16, 256),
            packed(2, 8, 8, 512),
            packed(7, 5, 4, 256),
            packed(2, 7, 5, 512),
            vmem((2, 2, 256, 128), F32),
            vmem((4, 4, 2, 256, 128), F32),
            dma((8,)), dma((8,)), dma((4,)), dma((8,)),
            dma((4,)), dma((4,)), dma((4,)), dma((8,)), dma((4,)),
        ],
        compiler_params=pltpu.CompilerParams(collective_id=0, vmem_limit_bytes=110 * 1024 * 1024),
    )(
        x.reshape(4, 4, 64, 1024),
        Wq,
        K_ext.reshape(4, 4, 64, 32, 128),
        V_ext.reshape(4, 4, 64, 32, 128),
        Wo,
    )
    return out.reshape(1, 1024, 1024)
```
